```python
import numpy as np

kernel_name = "dist_mean_ax1_xy_m4096_n1024"

def setup_inputs():
    return {"x": np.random.randn(8192, 2048).astype(np.float32)}

def reference(x: np.ndarray) -> np.ndarray:
    return np.mean(x, axis=1, keepdims=True)
```

```python
import jax
import jax.numpy as jnp
from jax import lax
from jax.experimental import pallas as pl
from jax.experimental.pallas import tpu as pltpu

LANES = 128
SUBLANES = 8

X_ROWS = 192
Y_ROWS = 192
S_ROWS = 112
SCHEDULE = (11, "relay", 9, 3, 1, "x_in", 2, 1, "side")
TAIL = (96, 32)


def _place_row_sums(buf, row0, rows, lane0, acc=None):
    tiles = [
        buf[pl.ds(row0, rows), c * LANES:(c + 1) * LANES]
        for c in range(buf.shape[1] // LANES)
    ]
    while len(tiles) > 1:
        tiles = [tiles[i] + tiles[i + 1] for i in range(0, len(tiles), 2)]
    sums = jnp.sum(tiles[0], axis=1, keepdims=True)
    shape = (SUBLANES, LANES)
    diag = lax.broadcasted_iota(jnp.int32, shape, 1) - lax.broadcasted_iota(
        jnp.int32, shape, 0
    )
    for r in range(0, rows, SUBLANES):
        acc = jnp.where(
            diag == lane0 + r, sums[r:r + SUBLANES], 0.0 if acc is None else acc
        )
    return acc


def pallas_dist_mean_ax1_xy_m4096_n1024_kernel(
x: jax.Array,
):
    m, n = x.shape
    n_blocks = m // LANES
    scale = 1.0 / (2 * n)
    side_rows = X_ROWS + Y_ROWS + S_ROWS
    side_blocks = pl.cdiv(side_rows, LANES)
    x_blocks = pl.cdiv(X_ROWS, LANES)
    chunks = [s for s in SCHEDULE if isinstance(s, int)]
    assert side_blocks + sum(chunks) == n_blocks - 1 and sum(TAIL) == LANES

    def kernel_body(x_hbm, o_ref, buf, part, recv, x_out, x_back, relay,
                    load_sems, send_sems, recv_sems, side_sems):
        def rows(ref, start, stop):
            return ref.at[pl.ds(start, stop - start)]

        bounds = [side_rows]
        for i in range(len(chunks)):
            bounds.append((side_blocks + sum(chunks[:i + 1])) * LANES)
        for t in TAIL:
            bounds.append(bounds[-1] + t)
        loads = [
            pltpu.make_async_copy(rows(x_hbm, a, b), rows(buf, a, b), load_sems.at[i])
            for i, (a, b) in enumerate(zip(bounds, bounds[1:]))
        ]
        s0 = X_ROWS + Y_ROWS
        relay_in = pltpu.make_async_copy(rows(x_hbm, s0, side_rows), relay, side_sems.at[0])
        relay_out = pltpu.make_async_copy(relay, rows(buf, s0, side_rows), side_sems.at[1])
        loads[0].start()
        relay_in.start()
        for load in loads[1:]:
            load.start()

        my_x, my_y = lax.axis_index("x"), lax.axis_index("y")
        x_peer, y_peer = (1 - my_x, my_y), (my_x, 1 - my_y)
        barrier = pltpu.get_barrier_semaphore()
        for peer in (y_peer, x_peer):
            pl.semaphore_signal(barrier, inc=1, device_id=peer,
                                device_id_type=pl.DeviceIdType.MESH)
        pl.semaphore_wait(barrier, 2)

        def push(src, dst, send_sem, recv_sem, peer):
            return pltpu.make_async_remote_copy(
                src, dst, send_sem, recv_sem, device_id=peer,
                device_id_type=pl.DeviceIdType.MESH)

        x_raw = push(rows(x_hbm, 0, X_ROWS), rows(buf, 0, X_ROWS),
                     side_sems.at[2], side_sems.at[3], x_peer)
        y_raw = push(rows(x_hbm, X_ROWS, s0), rows(buf, X_ROWS, s0),
                     side_sems.at[4], side_sems.at[5], y_peer)
        x_sums = push(x_out, x_back, side_sems.at[6], side_sems.at[7], x_peer)
        x_raw.start()
        y_raw.start()

        exchanges = []

        def exchange(b0, b1):
            k = len(exchanges)
            copy = push(rows(part, b0, b1), rows(recv, b0, b1),
                        send_sems.at[k], recv_sems.at[k], y_peer)
            copy.start()
            exchanges.append((copy, b0, b1))

        def reduce_blocks(dst, b0, b1):
            def reduce_block(b):
                row0 = b * LANES if isinstance(b, int) else pl.multiple_of(b * LANES, LANES)
                placed = _place_row_sums(buf, row0, LANES, 0)
                dst[pl.ds(b, 1), :] = jnp.sum(placed, axis=0, keepdims=True)

            if b1 - b0 == 1:
                reduce_block(b0)
            else:
                pl.loop(b0, b1)(reduce_block)

        pending = iter(loads)
        block = side_blocks
        for step in SCHEDULE:
            if step == "relay":
                relay_in.wait()
                relay_out.start()
            elif step == "x_in":
                x_raw.wait_recv()
                y_raw.wait_recv()
                reduce_blocks(x_out, 0, x_blocks)
                x_sums.start()
            elif step == "side":
                relay_out.wait()
                reduce_blocks(part, x_blocks, side_blocks)
                x_sums.wait_recv()
                shape = (x_blocks, LANES)
                row = (lax.broadcasted_iota(jnp.int32, shape, 0) * LANES
                       + lax.broadcasted_iota(jnp.int32, shape, 1))
                part[0:x_blocks, :] = jnp.where(row < X_ROWS, x_back[...], x_out[...])
                exchange(0, side_blocks)
            else:
                next(pending).wait()
                reduce_blocks(part, block, block + step)
                exchange(block, block + step)
                block += step

        placed, lane = None, 0
        for t in TAIL:
            next(pending).wait()
            placed = _place_row_sums(buf, m - LANES + lane, t, lane, placed)
            lane += t
        last = jnp.sum(placed, axis=0, keepdims=True)
        part[block:, :] = last
        exchange(block, n_blocks)

        for copy in (x_raw, y_raw, x_sums):
            copy.wait_send()
        for copy, b0, b1 in exchanges[:-1]:
            copy.wait()
            o_ref[b0:b1, :] = (part[b0:b1, :] + recv[b0:b1, :]) * scale
        exchanges[-1][0].wait()
        o_ref[block:, :] = (last + recv[block:, :]) * scale

    out = pl.pallas_call(
        kernel_body,
        out_shape=jax.ShapeDtypeStruct((n_blocks, LANES), jnp.float32),
        in_specs=[pl.BlockSpec(memory_space=pltpu.HBM)],
        out_specs=pl.BlockSpec(memory_space=pltpu.VMEM),
        scratch_shapes=[
            pltpu.VMEM((m, n), jnp.float32),
            pltpu.VMEM((n_blocks, LANES), jnp.float32),
            pltpu.VMEM((n_blocks, LANES), jnp.float32),
            pltpu.VMEM((x_blocks, LANES), jnp.float32),
            pltpu.VMEM((x_blocks, LANES), jnp.float32),
            pltpu.SMEM((S_ROWS, n), jnp.float32),
            pltpu.SemaphoreType.DMA((len(chunks) + len(TAIL),)),
            pltpu.SemaphoreType.DMA((len(chunks) + 2,)),
            pltpu.SemaphoreType.DMA((len(chunks) + 2,)),
            pltpu.SemaphoreType.DMA((8,)),
        ],
        compiler_params=pltpu.CompilerParams(
            vmem_limit_bytes=40 * 1024 * 1024,
            collective_id=0,
            disable_bounds_checks=True,
            disable_semaphore_checks=True,
        ),
    )(x)
    return out.reshape(m, 1)
```

```python
import jax
import jax.numpy as jnp
from jax import lax
from jax.experimental import pallas as pl
from jax.experimental.pallas import tpu as pltpu

LANES = 128
SUBLANES = 8
HEAD_BLOCKS = 2
PUSH_ROWS = 232
LATE_ROWS = 32


def _place_row_sums(ref, row0, rows, lane0, acc=0.0):
    tiles = [
        ref[pl.ds(row0, rows), c * LANES:(c + 1) * LANES]
        for c in range(ref.shape[1] // LANES)
    ]
    while len(tiles) > 1:
        tiles = [tiles[i] + tiles[i + 1] for i in range(0, len(tiles), 2)]
    sums = jnp.sum(tiles[0], axis=1, keepdims=True)
    shape = (SUBLANES, LANES)
    diag = lax.broadcasted_iota(jnp.int32, shape, 1) - lax.broadcasted_iota(
        jnp.int32, shape, 0
    )
    for r in range(0, rows, SUBLANES):
        acc = jnp.where(diag == lane0 + r, sums[r:r + SUBLANES], acc)
    return acc


def _to_lanes(placed):
    return jnp.sum(placed, axis=0, keepdims=True)


def pallas_dist_mean_ax1_xy_m4096_n1024_kernel(
x: jax.Array,
):
    m, n = x.shape
    n_blocks = m // LANES
    scale = 1.0 / (2 * n)
    body_blocks = n_blocks - HEAD_BLOCKS - 1
    passes = LANES // SUBLANES
    head_rows = HEAD_BLOCKS * LANES
    last = n_blocks - 1

    def kernel_body(x_hbm, o_ref, buf, pushed, placed, part, recv, late_out, late_in,
                    pass_sems, load_sems, send_sems, recv_sems):
        def rows(ref, start, stop):
            return ref.at[pl.ds(start, stop - start)]

        def body_pass(g):
            def view(ref):
                blocks = rows(ref, head_rows, last * LANES).reshape(body_blocks, LANES, n)
                return blocks.at[:, pl.ds(g * SUBLANES, SUBLANES)]

            return pltpu.make_async_copy(view(x_hbm), view(buf), pass_sems.at[g])

        def load(start, stop, k):
            return pltpu.make_async_copy(
                rows(x_hbm, start, stop), rows(buf, start, stop), load_sems.at[k])

        body_pass(0).start()
        my_x, my_y = lax.axis_index("x"), lax.axis_index("y")
        peer = (my_x, 1 - my_y)
        barrier = pltpu.get_barrier_semaphore()
        pl.semaphore_signal(barrier, inc=1, device_id=peer,
                            device_id_type=pl.DeviceIdType.MESH)
        if_giver, if_taker = pl.when(my_y == 1), pl.when(my_y == 0)

        head = load(0, PUSH_ROWS, 0)
        head_rest = load(PUSH_ROWS, head_rows, 1)
        tail = load(last * LANES, m - LATE_ROWS, 2)
        late = load(m - LATE_ROWS, m, 3)
        for g in range(1, passes):
            body_pass(g).start()
        head_rest.start()
        if_taker(head.start)
        tail.start()
        late.start()

        def send(src, dst, k):
            return pltpu.make_async_remote_copy(
                src, dst, send_sems.at[k], recv_sems.at[k], device_id=peer,
                device_id_type=pl.DeviceIdType.MESH)

        push = send(rows(x_hbm, 0, PUSH_ROWS), pushed, 0)
        body_sums = send(rows(part, HEAD_BLOCKS, last), rows(recv, HEAD_BLOCKS, last), 1)
        head_sums = send(rows(part, 0, HEAD_BLOCKS), rows(recv, 0, HEAD_BLOCKS), 2)
        tail_sums = send(rows(part, last, n_blocks), rows(recv, last, n_blocks), 3)
        late_sums = send(late_out, late_in, 4)

        pl.semaphore_wait(barrier, 1)
        if_giver(push.start)

        placed[...] = jnp.zeros_like(placed)

        @pl.loop(0, passes)
        def _(g):
            body_pass(g).wait()
            for j in range(body_blocks):
                row0 = pl.multiple_of(head_rows + j * LANES + g * SUBLANES, SUBLANES)
                placed[j] = _place_row_sums(buf, row0, SUBLANES, g * SUBLANES, placed[j])

        for j in range(body_blocks):
            part[pl.ds(HEAD_BLOCKS + j, 1), :] = _to_lanes(placed[j])
        body_sums.start()

        head_rest.wait()
        rest = _place_row_sums(buf, PUSH_ROWS, head_rows - PUSH_ROWS, PUSH_ROWS - LANES)

        @if_giver
        def _():
            part[0:1, :] = jnp.zeros((1, LANES), jnp.float32)
            part[1:2, :] = _to_lanes(rest)
            head_sums.start()

        tail.wait()
        tail_row = _to_lanes(_place_row_sums(buf, last * LANES, LANES - LATE_ROWS, 0))
        part[last:, :] = tail_row
        tail_sums.start()

        late.wait()
        late_row = _to_lanes(
            _place_row_sums(buf, m - LATE_ROWS, LATE_ROWS, LANES - LATE_ROWS))
        late_out[...] = late_row
        late_sums.start()

        @if_taker
        def _():
            head.wait()
            first = _place_row_sums(buf, 0, LANES, 0)
            second = _place_row_sums(buf, LANES, PUSH_ROWS - LANES, 0, rest)
            push.wait_recv()
            part[0:1, :] = _to_lanes(first + _place_row_sums(pushed, 0, LANES, 0))
            part[1:2, :] = _to_lanes(
                second + _place_row_sums(pushed, LANES, PUSH_ROWS - LANES, 0))
            head_sums.start()

        if_giver(push.wait_send)
        for copy, b0, b1 in ((body_sums, HEAD_BLOCKS, last), (head_sums, 0, HEAD_BLOCKS)):
            copy.wait()
            o_ref[b0:b1, :] = (part[b0:b1, :] + recv[b0:b1, :]) * scale
        late_sums.wait_send()
        tail_sums.wait()
        total = tail_row + late_row + recv[last:, :]
        lane = lax.broadcasted_iota(jnp.int32, (1, LANES), 1)
        late_sums.wait_recv()
        chains = [0.0] * 3
        for j in range(LANES - LATE_ROWS, LANES):
            chains[j % 3] = jnp.where(lane == j, late_in[0, j], chains[j % 3])
        for chain in chains:
            total = total + chain
        o_ref[last:, :] = total * scale

    out = pl.pallas_call(
        kernel_body,
        out_shape=jax.ShapeDtypeStruct((n_blocks, LANES), jnp.float32),
        in_specs=[pl.BlockSpec(memory_space=pltpu.HBM)],
        out_specs=pl.BlockSpec(memory_space=pltpu.VMEM),
        scratch_shapes=[
            pltpu.VMEM((m, n), jnp.float32),
            pltpu.VMEM((PUSH_ROWS, n), jnp.float32),
            pltpu.VMEM((body_blocks, SUBLANES, LANES), jnp.float32),
            pltpu.VMEM((n_blocks, LANES), jnp.float32),
            pltpu.VMEM((n_blocks, LANES), jnp.float32),
            pltpu.VMEM((1, LANES), jnp.float32),
            pltpu.SMEM((1, LANES), jnp.float32),
            pltpu.SemaphoreType.DMA((passes,)),
            pltpu.SemaphoreType.DMA((4,)),
            pltpu.SemaphoreType.DMA((5,)),
            pltpu.SemaphoreType.DMA((5,)),
        ],
        compiler_params=pltpu.CompilerParams(
            vmem_limit_bytes=40 * 1024 * 1024,
            collective_id=0,
            disable_bounds_checks=True,
            disable_semaphore_checks=True,
        ),
    )(x)
    return out.reshape(m, 1)
```

```python
import jax
import jax.numpy as jnp
from jax import lax
from jax.experimental import pallas as pl
from jax.experimental.pallas import tpu as pltpu

LANES = 128
SUBLANES = 8
BLOCK = LANES
HEAD = 2
PUSHED = 232
PIECE = 16
PHASE = 7
SPLIT = 20
LATE = 32


def _place_row_sums(ref, row0, rows, lane0, placed=0.0):
    shape = (SUBLANES, LANES)
    diag = lax.broadcasted_iota(jnp.int32, shape, 1) - lax.broadcasted_iota(
        jnp.int32, shape, 0
    )
    for i in range(0, rows, SUBLANES):
        group = ref[pl.ds(row0 + i, SUBLANES)]
        tiles = [group[t] for t in range(SUBLANES)]
        while len(tiles) > 1:
            tiles = [a + b for a, b in zip(tiles[::2], tiles[1::2])]
        sums = jnp.sum(tiles[0], axis=1, keepdims=True)
        placed = jnp.where(diag == lane0 + i, sums, placed)
    return placed


def _as_row(placed):
    return jnp.sum(placed, axis=0, keepdims=True)


def pallas_dist_mean_ax1_xy_m4096_n1024_kernel(
x: jax.Array,
):
    m, n = x.shape
    assert n == SUBLANES * LANES and m % BLOCK == 0
    n_blocks = m // BLOCK
    scale = 1.0 / (2 * n)
    last = n_blocks - 1
    body = last - HEAD
    passes = BLOCK // PIECE
    head_rows = HEAD * BLOCK
    body_start = head_rows + PHASE
    body_stop = body_start + body * BLOCK
    early = BLOCK - LATE

    def kernel_body(x_hbm, o_ref, buf, pushed, placed, part, recv, late_out,
                    late_in, relay, pass_sems, load_sems, send_sems, recv_sems):
        def span(ref, start, stop):
            return ref.at[pl.ds(start, stop - start)]

        def load(start, stop, k):
            return pltpu.make_async_copy(
                span(x_hbm, start, stop), span(buf, start, stop), load_sems.at[k])

        def load_pass(p, sem, start=0, stop=body):
            def pieces(ref):
                blocks = span(ref, body_start, body_stop).reshape(
                    body, BLOCK, SUBLANES, LANES)
                return blocks.at[pl.ds(start, stop - start), pl.ds(p * PIECE, PIECE)]

            return pltpu.make_async_copy(pieces(x_hbm), pieces(buf), sem)

        wrap_pass = load_pass(passes - 1, pass_sems.at[passes - 1])
        final_pass = [
            (load_pass(passes - 2, load_sems.at[k], start, stop), start, stop)
            for k, (start, stop) in enumerate(((0, SPLIT), (SPLIT, body)))
        ]
        fringe = load(head_rows, body_start, 2)
        head = load(0, PUSHED, 3)
        tail = load(body_stop, m - LATE, 4)
        late = load(m - LATE, m, 5)
        relay_in = pltpu.make_async_copy(
            span(x_hbm, PUSHED, head_rows), relay, load_sems.at[6])
        relay_out = pltpu.make_async_copy(
            relay, span(buf, PUSHED, head_rows), load_sems.at[7])

        wrap_pass.start()
        relay_in.start()
        my_x, my_y = lax.axis_index("x"), lax.axis_index("y")
        peer = (my_x, 1 - my_y)
        if_giver, if_taker = pl.when(my_y == 1), pl.when(my_y == 0)
        barrier = pltpu.get_barrier_semaphore()
        pl.semaphore_signal(barrier, inc=1, device_id=peer,
                            device_id_type=pl.DeviceIdType.MESH)
        fringe.start()
        for p in range(passes - 2):
            load_pass(p, pass_sems.at[p]).start()
        for copy, _, _ in final_pass:
            copy.start()
        if_taker(head.start)
        tail.start()
        late.start()

        def send(src, dst, k):
            return pltpu.make_async_remote_copy(
                src, dst, send_sems.at[k], recv_sems.at[k], device_id=peer,
                device_id_type=pl.DeviceIdType.MESH)

        push = send(span(x_hbm, 0, PUSHED), pushed, 0)
        head_sums = send(span(part, 0, HEAD), span(recv, 0, HEAD), 1)
        body_sums = send(span(part, HEAD, last), span(recv, HEAD, last), 2)
        tail_sums = send(span(part, last, n_blocks), span(recv, last, n_blocks), 3)
        late_sums = send(late_out, late_in, 4)

        pl.semaphore_wait(barrier, 1)
        if_giver(push.start)

        placed[...] = jnp.zeros_like(placed)
        wrap_pass.wait()
        fringe.wait()
        relay_in.wait()
        relay_out.start()

        @pl.loop(0, passes - 2)
        def _(p):
            load_pass(p, pass_sems.at[p]).wait()
            for j in range(body):
                placed[j] = _place_row_sums(
                    buf, (HEAD + j) * BLOCK + p * PIECE, PIECE, p * PIECE, placed[j])

        relay_out.wait()
        relayed = _place_row_sums(buf, PUSHED, head_rows - PUSHED, PUSHED - BLOCK)
        done = BLOCK - 2 * PIECE
        for copy, start, stop in final_pass:
            copy.wait()
            for j in range(start, stop):
                part[pl.ds(HEAD + j, 1), :] = _as_row(_place_row_sums(
                    buf, (HEAD + j) * BLOCK + done, 2 * PIECE, done, placed[j]))
        body_sums.start()

        @if_giver
        def _():
            part[0:1, :] = jnp.zeros((1, LANES), jnp.float32)
            part[1:2, :] = _as_row(relayed)
            head_sums.start()

        tail.wait()
        tail_row = _as_row(_place_row_sums(buf, last * BLOCK, early, 0))
        part[last:, :] = tail_row
        tail_sums.start()

        late.wait()
        late_row = _as_row(_place_row_sums(buf, m - LATE, LATE, early))
        late_out[...] = late_row
        late_sums.start()

        @if_taker
        def _():
            head.wait()
            first = _place_row_sums(buf, 0, BLOCK, 0)
            second = _place_row_sums(buf, BLOCK, PUSHED - BLOCK, 0, relayed)
            push.wait_recv()
            part[0:1, :] = _as_row(first + _place_row_sums(pushed, 0, BLOCK, 0))
            part[1:2, :] = _as_row(
                second + _place_row_sums(pushed, BLOCK, PUSHED - BLOCK, 0))
            head_sums.start()

        if_giver(push.wait_send)
        for copy, start, stop in ((body_sums, HEAD, last), (head_sums, 0, HEAD)):
            copy.wait()
            o_ref[start:stop, :] = (part[start:stop, :] + recv[start:stop, :]) * scale
        late_sums.wait_send()
        tail_sums.wait()
        total = tail_row + late_row + recv[last:, :]
        lane = lax.broadcasted_iota(jnp.int32, (1, LANES), 1)
        late_sums.wait_recv()
        chains = [0.0] * 3
        for j in range(early, LANES):
            chains[j % 3] = jnp.where(lane == j, late_in[0, j], chains[j % 3])
        for chain in chains:
            total = total + chain
        o_ref[last:, :] = total * scale

    tiles = (
        x.reshape(m // SUBLANES, SUBLANES, n // LANES, LANES)
        .transpose(0, 2, 1, 3)
        .reshape(m, SUBLANES, LANES)
    )
    out = pl.pallas_call(
        kernel_body,
        out_shape=jax.ShapeDtypeStruct((n_blocks, LANES), jnp.float32),
        in_specs=[pl.BlockSpec(memory_space=pltpu.HBM)],
        out_specs=pl.BlockSpec(memory_space=pltpu.VMEM),
        scratch_shapes=[
            pltpu.VMEM((m, SUBLANES, LANES), jnp.float32),
            pltpu.VMEM((PUSHED, SUBLANES, LANES), jnp.float32),
            pltpu.VMEM((body, SUBLANES, LANES), jnp.float32),
            pltpu.VMEM((n_blocks, LANES), jnp.float32),
            pltpu.VMEM((n_blocks, LANES), jnp.float32),
            pltpu.VMEM((1, LANES), jnp.float32),
            pltpu.SMEM((1, LANES), jnp.float32),
            pltpu.SMEM((head_rows - PUSHED, SUBLANES, LANES), jnp.float32),
            pltpu.SemaphoreType.DMA((passes,)),
            pltpu.SemaphoreType.DMA((8,)),
            pltpu.SemaphoreType.DMA((5,)),
            pltpu.SemaphoreType.DMA((5,)),
        ],
        compiler_params=pltpu.CompilerParams(
            vmem_limit_bytes=32 * 1024 * 1024,
            collective_id=0,
            disable_bounds_checks=True,
            disable_semaphore_checks=True,
        ),
    )(tiles)
    return out.reshape(m, 1)
```
